```python
import numpy as np

kernel_name = "dist_mean_ax0_shard0_i_m1024_n512"

def setup_inputs():
    return {"x": np.random.randn(4096, 512).astype(np.float32)}

def reference(x: np.ndarray) -> np.ndarray:
    return np.mean(x, axis=0, keepdims=True)
```

```python
import jax
import jax.numpy as jnp
from jax import lax
from jax.experimental import pallas as pl
from jax.experimental.pallas import tpu as pltpu

_N_DEV = 4
_ROW_CHUNKS = (512, 384, 112, 16)


def pallas_dist_mean_ax0_shard0_i_m1024_n512_kernel(x: jax.Array):
    m, n = x.shape
    assert sum(_ROW_CHUNKS) == m
    starts = [sum(_ROW_CHUNKS[:c]) for c in range(len(_ROW_CHUNKS))]

    def body(x_hbm, out_ref, x_vmem, mine_ref, recv_ref, load_sems, send_sem, recv_sem):
        loads = [
            pltpu.make_async_copy(
                x_hbm.at[pl.ds(start, rows)],
                x_vmem.at[pl.ds(start, rows)],
                load_sems.at[c],
            )
            for c, (start, rows) in enumerate(zip(starts, _ROW_CHUNKS))
        ]
        for load in loads:
            load.start()

        me = lax.axis_index("i")
        barrier = pltpu.get_barrier_semaphore()
        for d in (2, 1, 3):
            pl.semaphore_signal(
                barrier,
                1,
                device_id=((me + d) & (_N_DEV - 1),),
                device_id_type=pl.DeviceIdType.MESH,
            )

        acc = None
        for c, (start, rows) in enumerate(zip(starts, _ROW_CHUNKS)):
            if c == len(loads) - 1:
                pl.semaphore_wait(barrier, _N_DEV - 1)
            loads[c].wait()
            chunk = x_vmem[pl.ds(start, rows), :].reshape(rows // 8, 8, n)
            part = jnp.sum(chunk, axis=0)
            acc = part if acc is None else acc + part
        mine = jnp.sum(acc, axis=0, keepdims=True) * (1.0 / (m * _N_DEV))
        mine_ref[...] = mine

        sends = [
            pltpu.make_async_remote_copy(
                mine_ref,
                recv_ref.at[d - 1],
                send_sem,
                recv_sem,
                device_id=((me + d) & (_N_DEV - 1),),
                device_id_type=pl.DeviceIdType.MESH,
            )
            for d in (2, 1, 3)
        ]
        for send in sends:
            send.start()
        for send in sends:
            send.wait_send()
        pltpu.make_async_copy(recv_ref, recv_ref, recv_sem).wait()
        out_ref[...] = (mine + recv_ref[0]) + (recv_ref[1] + recv_ref[2])

    return pl.pallas_call(
        body,
        out_shape=jax.ShapeDtypeStruct((1, n), x.dtype),
        in_specs=[pl.BlockSpec(memory_space=pltpu.HBM)],
        out_specs=pl.BlockSpec(memory_space=pltpu.VMEM),
        scratch_shapes=[
            pltpu.VMEM((m, n), x.dtype),
            pltpu.VMEM((1, n), jnp.float32),
            pltpu.VMEM((_N_DEV - 1, 1, n), jnp.float32),
            pltpu.SemaphoreType.DMA((len(_ROW_CHUNKS),)),
            pltpu.SemaphoreType.DMA(()),
            pltpu.SemaphoreType.DMA(()),
        ],
        compiler_params=pltpu.CompilerParams(collective_id=0),
    )(x)
```

```python
import functools

import jax
import jax.numpy as jnp
from jax import lax
from jax.experimental import pallas as pl
from jax.experimental.pallas import tpu as pltpu

_N_DEV = 4
_SUBLANES, _LANES = 8, 128

_DIAGONAL = 2
_PEERS = (_DIAGONAL, 1, 3)
_LAST_TO_START, _ITS_HELPER = 2, 1

_FULL_ROWS = (512, 352)
_SPLIT_ROWS = (112, 16)
_FORWARDED_ROWS = 32


def _sum_row_groups(x):
    rows, n = x.shape
    return jnp.sum(x.reshape(rows // _SUBLANES, _SUBLANES, n), axis=0)


def _mean_kernel(
    x_hbm,
    out_ref,
    x_vmem,
    forwarded_ref,
    acc_ref,
    my_sum_ref,
    peer_sums_ref,
    load_sems,
    last_rows_sem,
    forward_send_sem,
    forward_recv_sem,
    send_sem,
    recv_sem,
):
    m, n = x_hbm.shape
    split_start, split_rows = sum(_FULL_ROWS), sum(_SPLIT_ROWS)
    all_cols, wide_cols, last_cols = (
        pl.ds(0, n),
        pl.ds(0, n - _LANES),
        pl.ds(n - _LANES, _LANES),
    )

    full_blocks = [
        (pl.ds(sum(_FULL_ROWS[:i]), rows), all_cols)
        for i, rows in enumerate(_FULL_ROWS)
    ]
    wide_block = (pl.ds(split_start, split_rows), wide_cols)
    last_blocks = [
        (pl.ds(split_start + sum(_SPLIT_ROWS[:i]), rows), last_cols)
        for i, rows in enumerate(_SPLIT_ROWS)
    ]
    blocks = [*full_blocks, wide_block, *last_blocks]
    loads = [
        pltpu.make_async_copy(x_hbm.at[block], x_vmem.at[block], load_sems.at[i])
        for i, block in enumerate(blocks)
    ]
    for load in loads:
        load.start()

    def sum_of_block(i):
        loads[i].wait()
        return _sum_row_groups(x_vmem[blocks[i]])

    me = lax.axis_index("i")
    last_rows = pl.ds(m - _FORWARDED_ROWS, _FORWARDED_ROWS)
    load_last_rows = pltpu.make_async_copy(
        x_hbm.at[last_rows], x_vmem.at[last_rows], last_rows_sem
    )
    pl.when(me != _LAST_TO_START)(load_last_rows.start)

    barrier = pltpu.get_barrier_semaphore()
    for k in _PEERS:
        pl.semaphore_signal(
            barrier, 1, device_id=(me ^ k,), device_id_type=pl.DeviceIdType.MESH
        )
    pl.semaphore_wait(barrier, len(_PEERS))

    forward_last_rows = pltpu.make_async_remote_copy(
        x_hbm.at[last_rows],
        forwarded_ref,
        forward_send_sem,
        forward_recv_sem,
        device_id=(_ITS_HELPER,),
        device_id_type=pl.DeviceIdType.MESH,
    )
    pl.when(me == _LAST_TO_START)(forward_last_rows.start)

    acc_ref[...] = functools.reduce(
        jnp.add, (sum_of_block(i) for i in range(len(full_blocks)))
    )

    @pl.when(me != _LAST_TO_START)
    def _():
        load_last_rows.wait()
        acc_ref[...] += _sum_row_groups(x_vmem[last_rows])

    @pl.when(me == _ITS_HELPER)
    def _():
        forward_last_rows.wait_recv()
        acc_ref[...] += _sum_row_groups(forwarded_ref[...])

    def send_my_sum(k, cols):
        send = pltpu.make_async_remote_copy(
            my_sum_ref.at[:, cols],
            peer_sums_ref.at[k - 1, :, cols],
            send_sem,
            recv_sem,
            device_id=(me ^ k,),
            device_id_type=pl.DeviceIdType.MESH,
        )
        send.start()
        return send

    wide_acc, last_acc = acc_ref[:, wide_cols], acc_ref[:, last_cols]
    wide_acc += sum_of_block(len(full_blocks))
    my_sum_ref[:, wide_cols] = jnp.sum(wide_acc, axis=0, keepdims=True)
    sends = [send_my_sum(_DIAGONAL, wide_cols)]
    for i in range(len(full_blocks) + 1, len(blocks)):
        last_acc += sum_of_block(i)
    my_sum_ref[:, last_cols] = jnp.sum(last_acc, axis=0, keepdims=True)
    sends += [
        send_my_sum(k, last_cols if k == _DIAGONAL else all_cols) for k in _PEERS
    ]

    pl.when(me == _LAST_TO_START)(forward_last_rows.wait_send)
    for send in sends:
        send.wait_send()
    pltpu.make_async_copy(peer_sums_ref, peer_sums_ref, recv_sem).wait()
    total = (my_sum_ref[...] + peer_sums_ref[0]) + (peer_sums_ref[1] + peer_sums_ref[2])
    out_ref[...] = total * (1.0 / (m * _N_DEV))


def pallas_dist_mean_ax0_shard0_i_m1024_n512_kernel(x: jax.Array):
    m, n = x.shape
    assert sum(_FULL_ROWS) + sum(_SPLIT_ROWS) + _FORWARDED_ROWS == m, x.shape
    assert n % _LANES == 0 and n > _LANES, x.shape
    n_loads = len(_FULL_ROWS) + 1 + len(_SPLIT_ROWS)

    def mean_kernel(*refs):
        pl.run_scoped(
            functools.partial(_mean_kernel, *refs),
            pltpu.SemaphoreType.DMA((n_loads,)),
            *[pltpu.SemaphoreType.DMA(())] * 5,
        )

    return pl.pallas_call(
        mean_kernel,
        out_shape=jax.ShapeDtypeStruct((1, n), x.dtype),
        in_specs=[pl.BlockSpec(memory_space=pltpu.HBM)],
        out_specs=pl.BlockSpec(memory_space=pltpu.VMEM),
        scratch_shapes=[
            pltpu.VMEM((m, n), x.dtype),
            pltpu.VMEM((_FORWARDED_ROWS, n), x.dtype),
            pltpu.VMEM((_SUBLANES, n), x.dtype),
            pltpu.VMEM((1, n), x.dtype),
            pltpu.VMEM((len(_PEERS), 1, n), x.dtype),
        ],
        compiler_params=pltpu.CompilerParams(collective_id=0),
    )(x)
```

```python
import functools

import jax
import jax.numpy as jnp
from jax import lax
from jax.experimental import pallas as pl
from jax.experimental.pallas import tpu as pltpu

_N_DEV = 4
_SUBLANES, _LANES = 8, 128

_DIAGONAL = 2
_PEERS = (_DIAGONAL, 1, 3)
_LAST_TO_START, _ITS_HELPER = 2, 1

_FULL_PIECES = (512, 320)
_WIDE_PIECES = (128, 32)
_NARROW_PIECES = (144, 16)
_TAIL_ROWS = 32


def _sum_row_groups(x):
    rows, columns = x.shape
    return jnp.sum(x.reshape(rows // _SUBLANES, _SUBLANES, columns), axis=0)


def _sum_row_groups_pairwise(x):
    parts = [x[row : row + _SUBLANES] for row in range(0, x.shape[0], _SUBLANES)]
    while len(parts) > 1:
        pairs = [parts[i] + parts[i + 1] for i in range(0, len(parts) - 1, 2)]
        parts = pairs + parts[2 * len(pairs) :]
    return parts[0]


def _mean_kernel(
    x_hbm,
    out_ref,
    full_ref,
    wide_ref,
    narrow_ref,
    tail_ref,
    forwarded_ref,
    acc_ref,
    my_sum_ref,
    peer_sums_ref,
    load_sems,
    tail_sem,
    forward_send_sem,
    forward_recv_sem,
    send_sem,
    recv_sem,
):
    m, n = x_hbm.shape
    all_cols = pl.ds(0, n)
    wide_cols = pl.ds(0, n - _LANES)
    narrow_cols = pl.ds(n - _LANES, _LANES)

    started = []

    def start_loads(first_row, cols, dst_ref, pieces):
        mine = []
        for i, rows in enumerate(pieces):
            start = sum(pieces[:i])
            dst = dst_ref.at[pl.ds(start, rows)]
            load = pltpu.make_async_copy(
                x_hbm.at[pl.ds(first_row + start, rows), cols],
                dst,
                load_sems.at[len(started)],
            )
            load.start()
            started.append(load)
            mine.append((load, dst))

        def landed():
            for load, dst in mine:
                load.wait()
                yield dst[...]

        return landed()

    split_row = sum(_FULL_PIECES)
    full_pieces = start_loads(0, all_cols, full_ref, _FULL_PIECES)
    wide_pieces = start_loads(split_row, wide_cols, wide_ref, _WIDE_PIECES)
    narrow_pieces = start_loads(split_row, narrow_cols, narrow_ref, _NARROW_PIECES)

    me = lax.axis_index("i")
    tail_hbm = x_hbm.at[pl.ds(m - _TAIL_ROWS, _TAIL_ROWS)]
    load_tail = pltpu.make_async_copy(tail_hbm, tail_ref, tail_sem)
    pl.when(me != _LAST_TO_START)(load_tail.start)

    barrier = pltpu.get_barrier_semaphore()
    for k in _PEERS:
        pl.semaphore_signal(
            barrier, 1, device_id=(me ^ k,), device_id_type=pl.DeviceIdType.MESH
        )
    pl.semaphore_wait(barrier, len(_PEERS))

    forward_tail = pltpu.make_async_remote_copy(
        tail_hbm,
        forwarded_ref,
        forward_send_sem,
        forward_recv_sem,
        device_id=(_ITS_HELPER,),
        device_id_type=pl.DeviceIdType.MESH,
    )
    pl.when(me == _LAST_TO_START)(forward_tail.start)

    acc_ref[...] = functools.reduce(jnp.add, map(_sum_row_groups, full_pieces))

    @pl.when(me != _LAST_TO_START)
    def _():
        load_tail.wait()
        acc_ref[...] += _sum_row_groups(tail_ref[...])

    @pl.when(me == _ITS_HELPER)
    def _():
        forward_tail.wait_recv()
        acc_ref[...] += _sum_row_groups(forwarded_ref[...])

    def send_my_sum(k, cols):
        send = pltpu.make_async_remote_copy(
            my_sum_ref.at[:, cols],
            peer_sums_ref.at[k - 1, :, cols],
            send_sem,
            recv_sem,
            device_id=(me ^ k,),
            device_id_type=pl.DeviceIdType.MESH,
        )
        send.start()
        return send

    wide_acc, narrow_acc = acc_ref[:, wide_cols], acc_ref[:, narrow_cols]
    for piece in wide_pieces:
        wide_acc += _sum_row_groups_pairwise(piece)
    my_sum_ref[:, wide_cols] = jnp.sum(wide_acc, axis=0, keepdims=True)
    sends = [send_my_sum(_DIAGONAL, wide_cols)]
    for piece in narrow_pieces:
        narrow_acc += _sum_row_groups_pairwise(piece)
    my_sum_ref[:, narrow_cols] = jnp.sum(narrow_acc, axis=0, keepdims=True)
    for k in _PEERS:
        sends.append(send_my_sum(k, narrow_cols if k == _DIAGONAL else all_cols))

    pl.when(me == _LAST_TO_START)(forward_tail.wait_send)
    for send in sends:
        send.wait_send()
    pltpu.make_async_copy(peer_sums_ref, peer_sums_ref, recv_sem).wait()
    total = (my_sum_ref[...] + peer_sums_ref[0]) + (peer_sums_ref[1] + peer_sums_ref[2])
    out_ref[...] = total * (1.0 / (m * _N_DEV))


def pallas_dist_mean_ax0_shard0_i_m1024_n512_kernel(x: jax.Array):
    m, n = x.shape
    full_rows, split_rows = sum(_FULL_PIECES), sum(_WIDE_PIECES)
    assert split_rows == sum(_NARROW_PIECES)
    assert full_rows + split_rows + _TAIL_ROWS == m, x.shape
    assert n % _LANES == 0 and n > _LANES, x.shape
    n_loads = len(_FULL_PIECES) + len(_WIDE_PIECES) + len(_NARROW_PIECES)

    def mean_kernel(*refs):
        pl.run_scoped(
            functools.partial(_mean_kernel, *refs),
            pltpu.SemaphoreType.DMA((n_loads,)),
            *[pltpu.SemaphoreType.DMA(())] * 5,
        )

    return pl.pallas_call(
        mean_kernel,
        out_shape=jax.ShapeDtypeStruct((1, n), x.dtype),
        in_specs=[pl.BlockSpec(memory_space=pltpu.HBM)],
        out_specs=pl.BlockSpec(memory_space=pltpu.VMEM),
        scratch_shapes=[
            pltpu.VMEM((full_rows, n), x.dtype),
            pltpu.VMEM((split_rows, n - _LANES), x.dtype),
            pltpu.VMEM((split_rows, _LANES), x.dtype),
            pltpu.VMEM((_TAIL_ROWS, n), x.dtype),
            pltpu.VMEM((_TAIL_ROWS, n), x.dtype),
            pltpu.VMEM((_SUBLANES, n), x.dtype),
            pltpu.VMEM((1, n), x.dtype),
            pltpu.VMEM((len(_PEERS), 1, n), x.dtype),
        ],
        compiler_params=pltpu.CompilerParams(collective_id=0),
    )(x)
```
